```python
import numpy as np

kernel_name = "dist_ag_xy_y_m256_n256"

def setup_inputs():
    return {"x": np.random.randn(512, 256).astype(np.float32)}

def reference(x: np.ndarray) -> np.ndarray:
    return x
```

```python
import jax, jax.numpy as jnp
from jax import lax
from jax.experimental import pallas as pl
from jax.experimental.pallas import tpu as pltpu
MESH = pl.DeviceIdType.MESH

def mk(chunks):
    offs = [sum(chunks[:i]) for i in range(len(chunks))]
    K = len(chunks)
    def f(x):
        m, n = x.shape
        def body(x_ref, o_ref, sb, rb, lsem, ssem, rsem):
            mx = lax.axis_index("x"); my = lax.axis_index("y")
            nb = (mx, 1 - my)
            bar = pltpu.get_barrier_semaphore()
            pl.semaphore_signal(bar, 1, device_id=nb, device_id_type=MESH)
            mine = pl.multiple_of(my * m, m); other = pl.multiple_of((1 - my) * m, m)
            loads = [pltpu.make_async_copy(x_ref.at[pl.ds(o, c)], o_ref.at[pl.ds(mine + o, c)], lsem.at[i]) for i, (o, c) in enumerate(zip(offs, chunks))]
            for l in loads: l.start()
            rd = [pltpu.make_async_remote_copy(sb.at[pl.ds(o, c)], rb.at[pl.ds(o, c)], ssem.at[i], rsem.at[i], device_id=nb, device_id_type=MESH) for i, (o, c) in enumerate(zip(offs, chunks))]
            for i, (o, c) in enumerate(zip(offs, chunks)):
                loads[i].wait()
                sb[pl.ds(o, c), :] = o_ref[pl.ds(mine + o, c), :].astype(jnp.bfloat16)
                if i == 0: pl.semaphore_wait(bar, 1)
                rd[i].start()
            for i, (o, c) in enumerate(zip(offs, chunks)):
                rd[i].wait_recv()
                o_ref[pl.ds(other + o, c), :] = rb[pl.ds(o, c), :].astype(jnp.float32)
            for r in rd: r.wait_send()
        return pl.pallas_call(body, out_shape=jax.ShapeDtypeStruct((2 * m, n), x.dtype),
            in_specs=[pl.BlockSpec(memory_space=pltpu.HBM)], out_specs=pl.BlockSpec(memory_space=pltpu.VMEM),
            scratch_shapes=[pltpu.VMEM((m, n), jnp.bfloat16), pltpu.VMEM((m, n), jnp.bfloat16),
                            pltpu.SemaphoreType.DMA((K,)), pltpu.SemaphoreType.DMA((K,)), pltpu.SemaphoreType.DMA((K,))],
            compiler_params=pltpu.CompilerParams(collective_id=0))(x)
    return f
pallas_dist_ag_xy_y_m256_n256_kernel = mk([64] * 4)
```

```python
import jax
import jax.numpy as jnp
from jax import lax
from jax.experimental import pallas as pl
from jax.experimental.pallas import tpu as pltpu

MESH = pl.DeviceIdType.MESH
H = 32


def pallas_dist_ag_xy_y_m256_n256_kernel(x: jax.Array):
    m, n = x.shape

    def body(x_ref, o_ref, sb, rb, lsem, ssem, fsem, rsem):
        mx = lax.axis_index("x")
        my = lax.axis_index("y")
        ynb, xnb = (mx, 1 - my), (1 - mx, my)
        low = my == 0
        mine = pl.multiple_of(my * m, m)
        other = pl.multiple_of((1 - my) * m, m)
        parts = [
            (pl.multiple_of(mx * H, H), H),
            (2 * H, m - 2 * H),
            (pl.multiple_of((1 - mx) * H, H), H),
        ]

        loads = [
            pltpu.make_async_copy(
                x_ref.at[pl.ds(o, c)], o_ref.at[pl.ds(mine + o, c)], lsem.at[i])
            for i, (o, c) in enumerate(parts)
        ]
        for load in loads:
            load.start()

        bar = pltpu.get_barrier_semaphore()
        pl.semaphore_signal(bar, 1, device_id=ynb, device_id_type=MESH)

        @pl.when(low)
        def _():
            pl.semaphore_signal(bar, 1, device_id=xnb, device_id_type=MESH)

        sends = [
            pltpu.make_async_remote_copy(
                sb.at[pl.ds(o, c)], rb.at[pl.ds(o, c)], ssem.at[i], rsem.at[i],
                device_id=ynb, device_id_type=MESH)
            for i, (o, c) in enumerate(parts)
        ]
        frows = rb.at[pl.ds(*parts[0])]
        forward = pltpu.make_async_remote_copy(
            frows, frows, fsem, rsem.at[2], device_id=xnb, device_id_type=MESH)

        def pack(o, c):
            sb[pl.ds(o, c), :] = o_ref[pl.ds(mine + o, c), :].astype(sb.dtype)

        def unpack(o, c):
            o_ref[pl.ds(other + o, c), :] = rb[pl.ds(o, c), :].astype(o_ref.dtype)

        loads[0].wait()
        pack(*parts[0])
        pl.semaphore_wait(bar, 1 + low.astype(jnp.int32))
        sends[0].start()
        loads[1].wait()
        pack(*parts[1])
        sends[1].start()
        loads[2].wait()

        @pl.when(low)
        def _():
            pack(*parts[2])
            sends[2].start()

        sends[0].wait_recv()

        @pl.when(low)
        def _():
            forward.start()

        unpack(*parts[0])
        sends[1].wait_recv()
        unpack(*parts[1])
        sends[2].wait_recv()
        unpack(*parts[2])
        sends[0].wait_send()
        sends[1].wait_send()

        @pl.when(low)
        def _():
            forward.wait_send()
            sends[2].wait_send()

    return pl.pallas_call(
        body,
        out_shape=jax.ShapeDtypeStruct((2 * m, n), x.dtype),
        in_specs=[pl.BlockSpec(memory_space=pltpu.HBM)],
        out_specs=pl.BlockSpec(memory_space=pltpu.VMEM),
        scratch_shapes=[
            pltpu.VMEM((m, n), jnp.bfloat16),
            pltpu.VMEM((m, n), jnp.bfloat16),
            pltpu.SemaphoreType.DMA((3,)),
            pltpu.SemaphoreType.DMA((3,)),
            pltpu.SemaphoreType.DMA,
            pltpu.SemaphoreType.DMA((3,)),
        ],
        compiler_params=pltpu.CompilerParams(collective_id=0),
    )(x)
```
